```python
import numpy as np

kernel_name = "dist_sort_i_m128_n64"

def setup_inputs():
    return {"x": np.random.randn(512, 64).astype(np.float32)}

def reference(x: np.ndarray) -> np.ndarray:
    return np.sort(x, axis=0)
```

```python
import jax
import jax.numpy as jnp
from jax import lax
from jax.experimental import pallas as pl
from jax.experimental.pallas import tpu as pltpu

F32 = jnp.float32
BF16 = jnp.bfloat16
MESH = pl.DeviceIdType.MESH

_SORT8 = (
    ((0, 2), (1, 3), (4, 6), (5, 7)),
    ((0, 4), (1, 5), (2, 6), (3, 7)),
    ((0, 1), (2, 3), (4, 5), (6, 7)),
    ((2, 4), (3, 5)),
    ((1, 4), (3, 6)),
    ((1, 2), (3, 4), (5, 6)),
)


def _iotas():
    lane = lax.broadcasted_iota(jnp.int32, (8, 128), 1)
    sub = lax.broadcasted_iota(jnp.int32, (8, 128), 0)
    return lane, sub


def _srot(x, k):
    return pltpu.roll(x, (8 - k) % 8, 0)


def _t_in(xs):
    lane, sub = _iotas()
    xs = xs[::-1]
    for k in range(3):
        m = (lane & (1 << k)) != 0
        xs = [jnp.where(m, _srot(x, 1 << k), x) for x in xs]
    a = (lane + sub) >> 3
    for k in range(3):
        m = (a & (1 << k)) != 0
        xs = [jnp.where(m, xs[(i + (1 << k)) % 8], xs[i]) for i in range(8)]
    return [pltpu.roll(x, 8 * i, 1, stride=1, stride_axis=0) for i, x in enumerate(xs)]


def _rot_label(g, t):
    for k in range(3):
        d = 1 << k
        m = (t & d) != 0
        cand = [g[j + d] if j + d < 8 else _srot(g[j + d - 8], 1) for j in range(8)]
        g = [jnp.where(m, cand[j], g[j]) for j in range(8)]
    for k in range(3):
        m = (t & (8 << k)) != 0
        g = [jnp.where(m, _srot(x, 1 << k), x) for x in g]
    return g


def _t_out(f):
    lane, sub = _iotas()
    g = _rot_label(f, lane)
    pos = (lane & 63) - 8 * sub
    out = []
    for j in range(8):
        x0 = pltpu.roll(g[j], j, 1, stride=8, stride_axis=0)
        x1 = pltpu.roll(g[j], j + 64, 1, stride=8, stride_axis=0)
        out.append(jnp.where(pos >= j, x0, x1))
    return _rot_label(out, lane + 1)


def _v_stage(xs, d, desc=False):
    xs = list(xs)
    for i in range(len(xs)):
        if i & d == 0:
            lo, hi = jnp.minimum(xs[i], xs[i + d]), jnp.maximum(xs[i], xs[i + d])
            xs[i], xs[i + d] = (hi, lo) if desc else (lo, hi)
    return xs


def _s_stage(xs, d, desc=False, mirror=False):
    _, sub = _iotas()
    upper = (sub & d) != 0
    out = []
    for i, x in enumerate(xs):
        p = xs[len(xs) - 1 - i] if mirror else x
        up = _srot(p, d)
        dn = up if d == 4 else _srot(p, 8 - d)
        if desc:
            out.append(jnp.where(upper, jnp.minimum(x, dn), jnp.maximum(x, up)))
        else:
            out.append(jnp.where(upper, jnp.maximum(x, dn), jnp.minimum(x, up)))
    return out


def _v_merge(xs, desc=False):
    for d in (4, 2, 1):
        xs = _v_stage(xs, d, desc)
    return xs


def _bmerge(xs, desc=False):
    for d in (4, 2, 1):
        xs = _s_stage(xs, d, desc)
    return _v_merge(xs, desc)


def _flip(xs, m):
    bits = jnp.where(m, jnp.int32(-(2 ** 31)), jnp.int32(0))
    return [pltpu.bitcast(pltpu.bitcast(x, jnp.int32) ^ bits, F32) for x in xs]


def _sort64_bitonic(xs):
    _, sub = _iotas()
    b4 = (sub & 2) != 0
    b5 = (sub & 4) != 0
    xs = _flip(xs, b4)
    for layer in _SORT8:
        for i, j in layer:
            xs[i], xs[j] = jnp.minimum(xs[i], xs[j]), jnp.maximum(xs[i], xs[j])
    xs = _v_merge(_s_stage(xs, 1, mirror=True))
    xs = _flip(xs, b4 != b5)
    xs = _v_merge(_s_stage(_s_stage(xs, 2), 1))
    return xs, b5


def _clamp(d, lo, hi):
    return [jnp.maximum(l, jnp.minimum(h, x)) for x, l, h in zip(d, lo, hi)]


def _rot64(xs):
    return [pltpu.roll(x, 64, 1) for x in xs]


def _mins(a, b):
    return [jnp.minimum(x, y) for x, y in zip(a, b)]


def _maxs(a, b):
    return [jnp.maximum(x, y) for x, y in zip(a, b)]


def _rows(v, n):
    return [v[8 * i:8 * i + 8, :] for i in range(n)]


def _body(x_hbm, o_ref, xv, send_b, recv_a, recv_b, send_s, recv_s, ext,
          ld_sem, send_sem, recv_sem, up_sem, go_sem):
    ld_hi = pltpu.make_async_copy(x_hbm.at[pl.ds(32, 32)], xv.at[pl.ds(32, 32)], ld_sem.at[0])
    ld_lo = pltpu.make_async_copy(x_hbm.at[pl.ds(0, 32)], xv.at[pl.ds(0, 32)], ld_sem.at[1])
    ld_hi.start()
    ld_lo.start()

    me = lax.axis_index("i")
    bar = pltpu.get_barrier_semaphore()

    def sig(sem, dev):
        pl.semaphore_signal(sem, inc=1, device_id=(dev,), device_id_type=MESH)

    def cp_a(dev):
        return pltpu.make_async_remote_copy(
            x_hbm.at[pl.ds(0, 32)], recv_a, send_sem.at[0], recv_sem.at[0],
            device_id=(dev,), device_id_type=MESH)

    def cp_b(dev):
        return pltpu.make_async_remote_copy(
            send_b, recv_b, send_sem.at[1], recv_sem.at[1],
            device_id=(dev,), device_id_type=MESH)

    def cp_s(src, dev):
        return pltpu.make_async_remote_copy(
            send_s, recv_s.at[src >> 1], send_sem.at[2 + (dev >> 1)], recv_sem.at[2 + (src >> 1)],
            device_id=(dev,), device_id_type=MESH)

    @pl.when(me == 2)
    def _():
        pl.semaphore_wait(bar, 3)
        cp_a(0).start()
        for d in (0, 1, 3):
            sig(up_sem.at[1], d)

    @pl.when(me == 0)
    def _():
        for d in (2, 1, 3):
            sig(bar, d)

    @pl.when((me & 1) == 1)
    def _():
        sig(bar, 2)
        pl.semaphore_wait(bar, 1)
        sig(up_sem.at[0], 0)

    ld_hi.wait()
    send_b[...] = xv[32:64, :].astype(BF16)

    @pl.when(me == 2)
    def _():
        cp_b(0).start()

    ld_lo.wait()
    lane, sub = _iotas()
    hi_half = lane >= 64
    a, b5 = _sort64_bitonic(_t_in(_rows(xv[...], 8)))
    a = _flip(_bmerge(_flip(a, b5 != hi_half)), hi_half)
    ax = _rot64(a)
    a_lo, a_hi = _mins(a, ax), _maxs(a, ax)
    wire = _bmerge([jnp.where(hi_half, l, h) for l, h in zip(a_lo, a_hi)], desc=True)
    send_s[...] = jnp.concatenate(wire, axis=0).astype(BF16)

    for k in (1, 3):
        @pl.when(me == k)
        def _(k=k):
            cp_s(k, 0).start()

    @pl.when(me == 2)
    def _():
        cp_s(2, 1).start()
        cp_s(2, 3).start()

    a_lo, a_hi = _bmerge(a_lo), _bmerge(a_hi)
    ext[0] = jnp.full((64, 128), -jnp.inf, F32)
    ext[5] = jnp.full((64, 128), jnp.inf, F32)

    @pl.when(me == 0)
    def _():
        pl.semaphore_wait(up_sem.at[0], 2)
        sig(go_sem, 1)
        sig(go_sem, 3)
        cp_s(0, 1).start()
        cp_s(0, 3).start()
        pl.semaphore_wait(up_sem.at[1], 1)
        cp_a(2).start()
        cp_b(2).start()

    for k in (1, 3):
        @pl.when(me == k)
        def _(k=k):
            pl.semaphore_wait(go_sem, 1)
            cp_a(4 - k).start()
            cp_b(4 - k).start()
            pl.semaphore_wait(up_sem.at[1], 1)
            cp_s(k, 2).start()

    def load_run(slot):
        own = _rows(recv_s[slot].astype(F32), 8)
        oth = _rot64(own)
        r0 = [jnp.where(hi_half, o, w) for w, o in zip(own, oth)]
        r1 = [jnp.where(hi_half, w, o) for w, o in zip(own, oth)]
        return r0, r1

    cp_s(0, 0).wait_recv()
    b0, b1 = load_run(0)
    lo0, lo1 = _mins(a_lo, b0), _mins(a_hi, b1)
    hi0, hi1 = _maxs(a_lo, b0), _maxs(a_hi, b1)
    for i, blk in enumerate((_mins(lo0, lo1), _maxs(lo0, lo1), _mins(hi0, hi1), _maxs(hi0, hi1))):
        ext[1 + i] = jnp.concatenate(_bmerge(blk), axis=0)

    cp_s(2, 0).wait_recv()
    c0, c1 = load_run(1)
    e = [_rows(ext[jnp.clip(2 * me - 3 + t, 0, 5)], 8) for t in range(6)]
    w = [[jnp.where(hi_half, y, x) for x, y in zip(e[t], e[t + 1])] for t in range(5)]
    u_lo, u_hi = _clamp(c0, w[1], w[3]), _clamp(c1, w[2], w[4])
    m1, m2 = _bmerge(_mins(u_lo, u_hi)), _bmerge(_maxs(u_lo, u_hi))
    m0 = _bmerge(_mins(_clamp(c0, w[0], w[2]), _clamp(c1, w[1], w[3])))

    cp_a(0).wait_send()
    cp_b(0).wait_send()
    cp_s(0, 0).wait_send()
    cp_s(0, 2).wait_send()

    cp_a(0).wait_recv()
    cp_b(0).wait_recv()
    d = _rows(recv_a[...], 4) + _rows(recv_b[...].astype(F32), 4)
    d, b5 = _sort64_bitonic(_t_in(d))
    d = _bmerge(_flip(d, b5), desc=True)
    dx = _rot64(d)
    n0 = _bmerge(_clamp(d, m0, m1))
    n1 = _bmerge(_clamp(d, m1, m2))
    f = _bmerge(_clamp(dx, n0, n1))
    g = _t_out(f)
    for j in range(8):
        o_ref[pl.ds(7 - j, 8, stride=8), :] = g[j]


def pallas_dist_sort_i_m128_n64_kernel(x: jax.Array):
    out_t = pl.pallas_call(
        _body,
        out_shape=jax.ShapeDtypeStruct((64, 128), F32),
        in_specs=[pl.BlockSpec(memory_space=pl.ANY)],
        out_specs=pl.BlockSpec(memory_space=pltpu.VMEM),
        scratch_shapes=[
            pltpu.VMEM((64, 128), F32),
            pltpu.VMEM((32, 128), BF16),
            pltpu.VMEM((32, 128), F32),
            pltpu.VMEM((32, 128), BF16),
            pltpu.VMEM((64, 128), BF16),
            pltpu.VMEM((2, 64, 128), BF16),
            pltpu.VMEM((6, 64, 128), F32),
            pltpu.SemaphoreType.DMA((2,)),
            pltpu.SemaphoreType.DMA((4,)),
            pltpu.SemaphoreType.DMA((4,)),
            pltpu.SemaphoreType.REGULAR((2,)),
            pltpu.SemaphoreType.REGULAR,
        ],
        compiler_params=pltpu.CompilerParams(collective_id=0, disable_bounds_checks=True, disable_semaphore_checks=True),
    )(x.T)
    return out_t.T
```

```python
import jax
import jax.numpy as jnp
from jax import lax
from jax.experimental import pallas as pl
from jax.experimental.pallas import tpu as pltpu

F32 = jnp.float32
BF16 = jnp.bfloat16
U32 = jnp.uint32

RAW = 24
CHUNKS = ((24, 40), (40, 56), (56, 64))
SLOT = {(3, 0): 0, (1, 0): 1, (1, 2): 0, (3, 2): 1,
        (0, 1): 0, (2, 1): 1, (0, 3): 0, (2, 3): 1}
SORT8 = ((0, 2), (1, 3), (4, 6), (5, 7), (0, 4), (1, 5), (2, 6), (3, 7),
         (0, 1), (2, 3), (4, 5), (6, 7), (2, 4), (3, 5), (1, 4), (3, 6),
         (1, 2), (3, 4), (5, 6))


def _iotas():
    lane = lax.broadcasted_iota(jnp.int32, (8, 128), 1)
    sub = lax.broadcasted_iota(jnp.int32, (8, 128), 0)
    return lane, sub


def _vregs(v):
    return [v[8 * i:8 * i + 8, :] for i in range(v.shape[0] // 8)]


def _srot(x, k):
    return pltpu.roll(x, (8 - k) % 8, 0)


def _negate(xs, m):
    sign = jnp.where(m, -1.0, 1.0).astype(F32)
    return [x * sign for x in xs]


def _rot_v(g, t):
    for d in (1, 2, 4):
        m = (t & d) != 0
        g = [jnp.where(m, g[(j + d) % 8], g[j]) for j in range(8)]
    return g


def _rot_s(g, t):
    for d in (1, 2, 4):
        m = (t & d) != 0
        g = [jnp.where(m, _srot(x, d), x) for x in g]
    return g


def _rot_s_flat(g, t):
    out = []
    for x in g:
        c = [x] + [_srot(x, k) for k in range(1, 8)]
        for d in (1, 2, 4):
            m = (t & d) != 0
            c = [jnp.where(m, b, a) for a, b in zip(c[0::2], c[1::2])]
        out.append(c[0])
    return out


def _to_lanes_a(xs):
    lane, sub = _iotas()
    return _negate(_rot_s(xs, lane), (sub & 2) != 0)


def _to_lanes_b(xs):
    lane, sub = _iotas()
    xs = _rot_v(xs, (lane + sub) >> 3)
    return [pltpu.roll(x, 8 * i, 1, stride=1, stride_axis=0) for i, x in enumerate(xs)]


def _to_rows_pattern(j):
    lane, sub = _iotas()
    c_hi = (j + 1 + lane) & 7
    c_lo = (sub + 1 + (lane >> 3)) & 7
    return (lane & 64) | (c_hi << 3) | c_lo


def _to_rows(f, pat):
    lane, _ = _iotas()
    g = _rot_v(f, -(lane >> 3))
    g = [jnp.take_along_axis(g[j], pat[j], axis=1, mode="promise_in_bounds") for j in range(8)]
    return _rot_v(_rot_s_flat(g, -1 - (lane >> 3)), -1 - lane)


def _v_stage(xs, d, desc=False):
    xs = list(xs)
    for i in range(8):
        if i & d == 0:
            lo, hi = jnp.minimum(xs[i], xs[i + d]), jnp.maximum(xs[i], xs[i + d])
            xs[i], xs[i + d] = (hi, lo) if desc else (lo, hi)
    return xs


def _v_merge(xs, desc=False):
    for d in (4, 2, 1):
        xs = _v_stage(xs, d, desc)
    return xs


def _s_stage(xs, d, desc=False, mirror=False, skew=False):
    lane, sub = _iotas()
    upper = ((sub - lane if skew else sub) & d) != 0
    out = []
    for i, x in enumerate(xs):
        p = xs[7 - i] if mirror else x
        up = _srot(p, d)
        dn = up if d == 4 else _srot(p, 8 - d)
        if desc:
            out.append(jnp.where(upper, jnp.minimum(x, dn), jnp.maximum(x, up)))
        else:
            out.append(jnp.where(upper, jnp.maximum(x, dn), jnp.minimum(x, up)))
    return out


def _swap(xs, d):
    _, sub = _iotas()
    upper = (sub & d) != 0
    xs = list(xs)
    for i in range(4):
        a, b = xs[i], xs[i + 4]
        xs[i] = jnp.where(upper, _srot(b, 8 - d), a)
        xs[i + 4] = jnp.where(upper, b, _srot(a, d))
    return xs


def _bmerge(xs, desc=False, skew=False):
    for d in (4, 2, 1):
        xs = _s_stage(xs, d, desc, skew=skew)
    return _v_merge(xs, desc)


def _sort64_desc(xs):
    _, sub = _iotas()
    p0 = (sub & 1) != 0
    p1 = (sub & 2) != 0
    xs = list(xs)
    for i, j in SORT8:
        xs[i], xs[j] = jnp.minimum(xs[i], xs[j]), jnp.maximum(xs[i], xs[j])
    xs = _v_merge(_s_stage(xs, 4, mirror=True))
    xs = _negate(xs, p1 != p0)
    for d in (2, 4):
        xs = _v_stage(_swap(xs, d), 4)
    xs = _v_merge(_swap(xs, 2))
    xs = _negate(xs, p0)
    for d in (1, 4, 2):
        xs = _v_stage(_swap(xs, d), 4, True)
    return _v_merge(_swap(xs, 1), True)


def _clamp(run, lo, hi):
    return [jnp.maximum(l, jnp.minimum(h, x)) for x, l, h in zip(run, lo, hi)]


def _insert(blocks, run, first=False, last=False):
    out = []
    if first:
        out.append(_bmerge([jnp.minimum(x, h) for x, h in zip(run, blocks[0])]))
    for lo, hi in zip(blocks[:-1], blocks[1:]):
        out.append(_bmerge(_clamp(run, lo, hi)))
    if last:
        out.append(_bmerge([jnp.maximum(x, l) for x, l in zip(run, blocks[-1])]))
    return out


def _other_half(xs):
    return [pltpu.roll(x, 64, 1) for x in xs]


def _pack(xs):
    u = [lax.bitcast_convert_type(x, U32) for x in xs]
    return [a | (b >> 16) for a, b in zip(u[0::2], u[1::2])]


def _unpack(ws):
    out = []
    for w in ws:
        out.append(lax.bitcast_convert_type(w & U32(0xFFFF0000), F32))
        out.append(lax.bitcast_convert_type(w << 16, F32))
    return out


def _body(x_hbm, o_ref, xv, send_b, recv_a, recv_b, send_s, recv_s, ext, win, pat,
          ld_sem, send_sem, recv_sem, up_sem, go_sem):
    me = lax.axis_index("i")
    bar = pltpu.get_barrier_semaphore()
    nc = len(CHUNKS)

    def load(lo, hi, i):
        rows = pl.ds(lo, hi - lo)
        return pltpu.make_async_copy(x_hbm.at[rows], xv.at[rows], ld_sem.at[i])

    def signal(sem, dev):
        pl.semaphore_signal(sem, inc=1, device_id=(dev,), device_id_type=pl.DeviceIdType.MESH)

    def remote(src, dst, s, r, dev):
        return pltpu.make_async_remote_copy(
            src, dst, send_sem.at[s], recv_sem.at[r],
            device_id=(dev,), device_id_type=pl.DeviceIdType.MESH)

    def cp_raw(dev):
        return remote(x_hbm.at[pl.ds(0, RAW)], recv_a, 0, 0, dev)

    def cp_chunk(dev, i):
        rows = pl.ds(CHUNKS[i][0] - RAW, CHUNKS[i][1] - CHUNKS[i][0])
        return remote(send_b.at[rows], recv_b.at[rows], 3, 3 + i, dev)

    def cp_sorted(src, dev):
        slot = SLOT[(src, dev)]
        return remote(send_s, recv_s.at[slot], 1 + (dev >> 1), 1 + slot, dev)

    def send_diagonal(dev):
        cp_raw(dev).start()
        for i in range(nc):
            cp_chunk(dev, i).start()

    def put(ref, i, block):
        ref[i] = jnp.concatenate(block, axis=0)

    for i, (lo, hi) in enumerate(CHUNKS):
        load(lo, hi, 1 + i).start()

    @pl.when(me == 2)
    def _():
        pl.semaphore_wait(bar, 1)
        cp_raw(0).start()
        signal(up_sem.at[1], 0)

    load(0, RAW, 0).start()

    @pl.when(me == 0)
    def _():
        for dev in (2, 1, 3):
            signal(bar, dev)

    @pl.when((me & 1) == 1)
    def _():
        pl.semaphore_wait(bar, 1)
        signal(up_sem.at[0], 0)

    for i, (lo, hi) in enumerate(CHUNKS):
        load(lo, hi, 1 + i).wait()
        rows = xv[lo:hi, :]
        if i == nc - 1:
            rows = jnp.concatenate(_to_lanes_a(_vregs(rows)), axis=0)
        send_b[lo - RAW:hi - RAW, :] = rows.astype(BF16)

        @pl.when(me == 2)
        def _(i=i):
            cp_chunk(0, i).start()

    load(0, RAW, 0).wait()
    own = _sort64_desc(_to_lanes_b(_to_lanes_a(_vregs(xv[...]))))
    send_s[...] = jnp.concatenate(own, axis=0).astype(BF16)

    for k in (1, 3):
        @pl.when(me == k)
        def _(k=k):
            cp_sorted(k, 0).start()

    mine = _insert([_bmerge(own)], _other_half(own), True, True)
    for j in range(8):
        pat[j] = _to_rows_pattern(j)
    lane, _ = _iotas()
    hi_half = lane >= 64

    @pl.when(me == 0)
    def _():
        pl.semaphore_wait(up_sem.at[0], 2)
        signal(bar, 2)
        signal(go_sem, 1)
        signal(go_sem, 3)
        cp_sorted(0, 1).start()
        cp_sorted(0, 3).start()
        pl.semaphore_wait(up_sem.at[1], 1)
        signal(up_sem.at[1], 1)
        signal(up_sem.at[1], 3)
        send_diagonal(2)

        cp_sorted(3, 0).wait_recv()
        cp_sorted(1, 0).wait_recv()
        b = _vregs(recv_s[0].astype(F32))
        c = _vregs(recv_s[1].astype(F32))
        st = mine
        for run in (b, c, _other_half(b), _other_half(c)):
            st = _insert(st, run, first=True)
        neg_inf = jnp.full((8, 128), -jnp.inf, F32)
        put(win, 0, [neg_inf] * 8)
        put(win, 1, [jnp.where(hi_half, x, neg_inf) for x in st[0]])
        put(win, 2, [jnp.where(hi_half, y, x) for x, y in zip(*st)])

    @pl.when(me != 0)
    def _():
        ext[0] = jnp.full((64, 128), -jnp.inf, F32)
        ext[5] = jnp.full((64, 128), jnp.inf, F32)
        for k in (1, 3):
            @pl.when(me == k)
            def _(k=k):
                pl.semaphore_wait(go_sem, 1)
                send_diagonal(4 - k)

        @pl.when(me == 2)
        def _():
            pl.semaphore_wait(bar, 1)
            cp_sorted(2, 1).start()
            cp_sorted(2, 3).start()

        cp_sorted(3, 0).wait_recv()
        b = _vregs(recv_s[0].astype(F32))
        st = _insert(_insert(mine, b, True, True), _other_half(b), True, True)
        for i, block in enumerate(st):
            put(ext, 1 + i, block)
        e = [_vregs(ext[jnp.clip(2 * me - 3 + t, 0, 5)]) for t in range(6)]
        st = [[jnp.where(hi_half, y, x) for x, y in zip(e[t], e[t + 1])] for t in range(5)]

        for k in (1, 3):
            @pl.when(me == k)
            def _(k=k):
                pl.semaphore_wait(up_sem.at[1], 1)
                cp_sorted(k, 2).start()

        cp_sorted(1, 0).wait_recv()
        c = _vregs(recv_s[1].astype(F32))
        st = _insert(_insert(st, c), _other_half(c))
        for i, block in enumerate(st):
            put(win, i, block)

    cp_raw(0).wait_recv()
    d = _to_lanes_a(_vregs(recv_a[...].astype(BF16).astype(F32)))
    cp_sorted(1, 0).wait_send()
    cp_sorted(1, 2).wait_send()
    cp_raw(0).wait_send()
    for i, (lo, hi) in enumerate(CHUNKS):
        if i == nc - 1:
            pltpu.make_async_copy(send_b, send_b, send_sem.at[3]).wait()
        cp_chunk(0, i).wait_recv()
        rows = _vregs(recv_b[lo - RAW:hi - RAW, :].astype(F32))
        d = d + (rows if i == nc - 1 else _to_lanes_a(rows))

    w = _pack(_sort64_desc(_to_lanes_b(d)))
    far = _unpack(_other_half(w))
    n0, n1 = _insert([_vregs(win[i]) for i in range(3)], _unpack(w))
    res = _to_rows(_bmerge(_clamp(far, n0, n1), desc=True, skew=True), pat)
    for j in range(8):
        o_ref[8 * j:8 * j + 8, :] = res[j]


def pallas_dist_sort_i_m128_n64_kernel(x: jax.Array):
    nc = len(CHUNKS)
    out_t = pl.pallas_call(
        _body,
        out_shape=jax.ShapeDtypeStruct((64, 128), F32),
        in_specs=[pl.BlockSpec(memory_space=pl.ANY)],
        out_specs=pl.BlockSpec(memory_space=pltpu.VMEM),
        scratch_shapes=[
            pltpu.VMEM((64, 128), F32),
            pltpu.VMEM((64 - RAW, 128), BF16),
            pltpu.VMEM((RAW, 128), F32),
            pltpu.VMEM((64 - RAW, 128), BF16),
            pltpu.VMEM((64, 128), BF16),
            pltpu.VMEM((2, 64, 128), BF16),
            pltpu.VMEM((6, 64, 128), F32),
            pltpu.VMEM((3, 64, 128), F32),
            pltpu.VMEM((8, 8, 128), jnp.int32),
            pltpu.SemaphoreType.DMA((1 + nc,)),
            pltpu.SemaphoreType.DMA((4,)),
            pltpu.SemaphoreType.DMA((3 + nc,)),
            pltpu.SemaphoreType.REGULAR((2,)),
            pltpu.SemaphoreType.REGULAR,
        ],
        compiler_params=pltpu.CompilerParams(
            collective_id=0, disable_bounds_checks=True, disable_semaphore_checks=True),
    )(x.T)
    return out_t.T
```

```python
import jax
import jax.numpy as jnp
from jax import lax
from jax.experimental import pallas as pl
from jax.experimental.pallas import tpu as pltpu

F32 = jnp.float32
BF16 = jnp.bfloat16
U32 = jnp.uint32

RAW = 24
CHUNKS = ((24, 40), (40, 56), (56, 64))
SLOT = {(3, 0): 0, (1, 0): 1, (1, 2): 0, (3, 2): 1,
        (0, 1): 0, (2, 1): 1, (0, 3): 0, (2, 3): 1}
SORT8 = ((0, 2), (1, 3), (4, 6), (5, 7), (0, 4), (1, 5), (2, 6), (3, 7),
         (0, 1), (2, 3), (4, 5), (6, 7), (2, 4), (3, 5), (1, 4), (3, 6),
         (1, 2), (3, 4), (5, 6))


def _iotas():
    lane = lax.broadcasted_iota(jnp.int32, (8, 128), 1)
    sub = lax.broadcasted_iota(jnp.int32, (8, 128), 0)
    return lane, sub


def _vregs(v):
    return [v[8 * i:8 * i + 8, :] for i in range(v.shape[0] // 8)]


def _srot(x, k):
    return pltpu.roll(x, (8 - k) % 8, 0)


def _negate(xs, m):
    sign = jnp.where(m, -1.0, 1.0).astype(F32)
    return [x * sign for x in xs]


def _rot_v(g, t):
    for d in (1, 2, 4):
        m = (t & d) != 0
        g = [jnp.where(m, g[(j + d) % 8], g[j]) for j in range(8)]
    return g


def _rot_s(g, t):
    for d in (1, 2, 4):
        m = (t & d) != 0
        g = [jnp.where(m, _srot(x, d), x) for x in g]
    return g


def _rot_s_flat(g, t):
    out = []
    for x in g:
        c = [x] + [_srot(x, k) for k in range(1, 8)]
        for d in (1, 2, 4):
            m = (t & d) != 0
            c = [jnp.where(m, b, a) for a, b in zip(c[0::2], c[1::2])]
        out.append(c[0])
    return out


def _to_lanes_a(xs):
    lane, sub = _iotas()
    return _negate(_rot_s(xs, lane), (sub & 2) != 0)


def _to_lanes_b(xs):
    lane, sub = _iotas()
    xs = _rot_v(xs, (lane + sub) >> 3)
    return [pltpu.roll(x, 8 * i, 1, stride=1, stride_axis=0) for i, x in enumerate(xs)]


def _to_rows_pattern(j):
    lane, sub = _iotas()
    c_hi = (j + 1 + lane) & 7
    c_lo = (sub + 1 + (lane >> 3)) & 7
    return (lane & 64) | (c_hi << 3) | c_lo


def _to_rows(f, pat):
    lane, _ = _iotas()
    g = _rot_v(f, -(lane >> 3))
    g = [jnp.take_along_axis(g[j], pat[j], axis=1, mode="promise_in_bounds") for j in range(8)]
    return _rot_v(_rot_s_flat(g, -1 - (lane >> 3)), -1 - lane)


def _v_stage(xs, d, desc=False):
    xs = list(xs)
    for i in range(8):
        if i & d == 0:
            lo, hi = jnp.minimum(xs[i], xs[i + d]), jnp.maximum(xs[i], xs[i + d])
            xs[i], xs[i + d] = (hi, lo) if desc else (lo, hi)
    return xs


def _v_merge(xs, desc=False):
    for d in (4, 2, 1):
        xs = _v_stage(xs, d, desc)
    return xs


def _s_stage(xs, d, desc=False, mirror=False, skew=False):
    lane, sub = _iotas()
    upper = ((sub - lane if skew else sub) & d) != 0
    out = []
    for i, x in enumerate(xs):
        p = xs[7 - i] if mirror else x
        up = _srot(p, d)
        dn = up if d == 4 else _srot(p, 8 - d)
        if desc:
            out.append(jnp.where(upper, jnp.minimum(x, dn), jnp.maximum(x, up)))
        else:
            out.append(jnp.where(upper, jnp.maximum(x, dn), jnp.minimum(x, up)))
    return out


def _swap(xs, d):
    _, sub = _iotas()
    upper = (sub & d) != 0
    xs = list(xs)
    for i in range(4):
        a, b = xs[i], xs[i + 4]
        xs[i] = jnp.where(upper, _srot(b, 8 - d), a)
        xs[i + 4] = jnp.where(upper, b, _srot(a, d))
    return xs


def _bmerge(xs, desc=False, skew=False):
    for d in (4, 2, 1):
        xs = _s_stage(xs, d, desc, skew=skew)
    return _v_merge(xs, desc)


def _sort64_desc(xs):
    _, sub = _iotas()
    p0 = (sub & 1) != 0
    p1 = (sub & 2) != 0
    xs = list(xs)
    for i, j in SORT8:
        xs[i], xs[j] = jnp.minimum(xs[i], xs[j]), jnp.maximum(xs[i], xs[j])
    xs = _v_merge(_s_stage(xs, 4, mirror=True))
    xs = _negate(xs, p1 != p0)
    for d in (2, 4):
        xs = _v_stage(_swap(xs, d), 4)
    xs = _v_merge(_swap(xs, 2))
    xs = _negate(xs, p0)
    for d in (1, 4, 2):
        xs = _v_stage(_swap(xs, d), 4, True)
    return _v_merge(_swap(xs, 1), True)


def _clamp(run, lo, hi):
    return [jnp.maximum(l, jnp.minimum(h, x)) for x, l, h in zip(run, lo, hi)]


def _insert(blocks, run, first=False, last=False):
    out = []
    if first:
        out.append(_bmerge([jnp.minimum(x, h) for x, h in zip(run, blocks[0])]))
    for lo, hi in zip(blocks[:-1], blocks[1:]):
        out.append(_bmerge(_clamp(run, lo, hi)))
    if last:
        out.append(_bmerge([jnp.maximum(x, l) for x, l in zip(run, blocks[-1])]))
    return out


def _other_half(xs):
    return [pltpu.roll(x, 64, 1) for x in xs]


def _pack(xs):
    u = [lax.bitcast_convert_type(x, U32) for x in xs]
    return [a | (b >> 16) for a, b in zip(u[0::2], u[1::2])]


def _unpack(ws):
    out = []
    for w in ws:
        out.append(lax.bitcast_convert_type(w & U32(0xFFFF0000), F32))
        out.append(lax.bitcast_convert_type(w << 16, F32))
    return out


def _body(x_hbm, o_ref, xv, send_b, recv_a, recv_b, send_s, recv_s, ext, win, pat,
          ld_sem, send_sem, recv_sem, up_sem, go_sem):
    me = lax.axis_index("i")
    bar = pltpu.get_barrier_semaphore()
    nc = len(CHUNKS)

    def load(lo, hi, i):
        rows = pl.ds(lo, hi - lo)
        return pltpu.make_async_copy(x_hbm.at[rows], xv.at[rows], ld_sem.at[i])

    def signal(sem, dev):
        pl.semaphore_signal(sem, inc=1, device_id=(dev,), device_id_type=pl.DeviceIdType.MESH)

    def remote(src, dst, s, r, dev):
        return pltpu.make_async_remote_copy(
            src, dst, send_sem.at[s], recv_sem.at[r],
            device_id=(dev,), device_id_type=pl.DeviceIdType.MESH)

    def cp_raw(dev):
        return remote(x_hbm.at[pl.ds(0, RAW)], recv_a, 0, 0, dev)

    def cp_chunk(dev, i):
        rows = pl.ds(CHUNKS[i][0] - RAW, CHUNKS[i][1] - CHUNKS[i][0])
        return remote(send_b.at[rows], recv_b.at[rows], 3, 3 + i, dev)

    def cp_sorted(src, dev):
        slot = SLOT[(src, dev)]
        return remote(send_s, recv_s.at[slot], 1 + (dev >> 1), 1 + slot, dev)

    def send_diagonal(dev):
        cp_raw(dev).start()
        for i in range(nc):
            cp_chunk(dev, i).start()

    def put(ref, i, block):
        ref[i] = jnp.concatenate(block, axis=0)

    load(*CHUNKS[0], 1).start()

    @pl.when(me == 2)
    def _():
        pl.semaphore_wait(bar, 1)
        cp_raw(0).start()
        signal(up_sem.at[1], 0)

    for i in range(1, nc):
        load(*CHUNKS[i], 1 + i).start(priority=1)

    @pl.when(me != 2)
    def _():
        load(0, RAW, 0).start()

    @pl.when(me == 0)
    def _():
        for dev in (2, 1, 3):
            signal(bar, dev)

    @pl.when((me & 1) == 1)
    def _():
        pl.semaphore_wait(bar, 1)
        signal(up_sem.at[0], 0)

    for i, (lo, hi) in enumerate(CHUNKS):
        load(lo, hi, 1 + i).wait()
        rows = xv[lo:hi, :]
        if i == nc - 1:
            rows = jnp.concatenate(_to_lanes_a(_vregs(rows)), axis=0)
        send_b[lo - RAW:hi - RAW, :] = rows.astype(BF16)

        @pl.when(me == 2)
        def _(i=i):
            cp_chunk(0, i).start()

    @pl.when(me == 2)
    def _():
        load(0, RAW, 0).start()

    load(0, RAW, 0).wait()
    own = _sort64_desc(_to_lanes_b(_to_lanes_a(_vregs(xv[...]))))
    send_s[...] = jnp.concatenate(own, axis=0).astype(BF16)

    for k in (1, 3):
        @pl.when(me == k)
        def _(k=k):
            cp_sorted(k, 0).start()

    mine = _insert([_bmerge(own)], _other_half(own), True, True)
    for j in range(8):
        pat[j] = _to_rows_pattern(j)
    lane, _ = _iotas()
    hi_half = lane >= 64

    @pl.when(me == 0)
    def _():
        pl.semaphore_wait(up_sem.at[0], 2)
        signal(bar, 2)
        signal(go_sem, 1)
        signal(go_sem, 3)
        cp_sorted(0, 1).start()
        cp_sorted(0, 3).start()
        pl.semaphore_wait(up_sem.at[1], 1)
        signal(up_sem.at[1], 1)
        signal(up_sem.at[1], 3)
        send_diagonal(2)

        cp_sorted(3, 0).wait_recv()
        cp_sorted(1, 0).wait_recv()
        b = _vregs(recv_s[0].astype(F32))
        c = _vregs(recv_s[1].astype(F32))
        st = mine
        for run in (b, c, _other_half(b), _other_half(c)):
            st = _insert(st, run, first=True)
        neg_inf = jnp.full((8, 128), -jnp.inf, F32)
        put(win, 0, [neg_inf] * 8)
        put(win, 1, [jnp.where(hi_half, x, neg_inf) for x in st[0]])
        put(win, 2, [jnp.where(hi_half, y, x) for x, y in zip(*st)])

    @pl.when(me != 0)
    def _():
        ext[0] = jnp.full((64, 128), -jnp.inf, F32)
        ext[5] = jnp.full((64, 128), jnp.inf, F32)
        for k in (1, 3):
            @pl.when(me == k)
            def _(k=k):
                pl.semaphore_wait(go_sem, 1)
                send_diagonal(4 - k)

        @pl.when(me == 2)
        def _():
            pl.semaphore_wait(bar, 1)
            cp_sorted(2, 1).start()
            cp_sorted(2, 3).start()

        cp_sorted(3, 0).wait_recv()
        b = _vregs(recv_s[0].astype(F32))
        st = _insert(_insert(mine, b, True, True), _other_half(b), True, True)
        for i, block in enumerate(st):
            put(ext, 1 + i, block)
        e = [_vregs(ext[jnp.clip(2 * me - 3 + t, 0, 5)]) for t in range(6)]
        st = [[jnp.where(hi_half, y, x) for x, y in zip(e[t], e[t + 1])] for t in range(5)]

        for k in (1, 3):
            @pl.when(me == k)
            def _(k=k):
                pl.semaphore_wait(up_sem.at[1], 1)
                cp_sorted(k, 2).start()

        cp_sorted(1, 0).wait_recv()
        c = _vregs(recv_s[1].astype(F32))
        st = _insert(_insert(st, c), _other_half(c))
        for i, block in enumerate(st):
            put(win, i, block)

    cp_raw(0).wait_recv()
    d = _to_lanes_a(_vregs(recv_a[...].astype(BF16).astype(F32)))
    cp_sorted(1, 0).wait_send()
    cp_sorted(1, 2).wait_send()
    cp_raw(0).wait_send()
    for i, (lo, hi) in enumerate(CHUNKS):
        if i == nc - 1:
            pltpu.make_async_copy(send_b, send_b, send_sem.at[3]).wait()
        cp_chunk(0, i).wait_recv()
        rows = _vregs(recv_b[lo - RAW:hi - RAW, :].astype(F32))
        d = d + (rows if i == nc - 1 else _to_lanes_a(rows))

    w = _pack(_sort64_desc(_to_lanes_b(d)))
    far = _unpack(_other_half(w))
    n0, n1 = _insert([_vregs(win[i]) for i in range(3)], _unpack(w))
    res = _to_rows(_bmerge(_clamp(far, n0, n1), desc=True, skew=True), pat)
    for j in range(8):
        o_ref[8 * j:8 * j + 8, :] = res[j]


def pallas_dist_sort_i_m128_n64_kernel(x: jax.Array):
    nc = len(CHUNKS)
    out_t = pl.pallas_call(
        _body,
        out_shape=jax.ShapeDtypeStruct((64, 128), F32),
        in_specs=[pl.BlockSpec(memory_space=pl.ANY)],
        out_specs=pl.BlockSpec(memory_space=pltpu.VMEM),
        scratch_shapes=[
            pltpu.VMEM((64, 128), F32),
            pltpu.VMEM((64 - RAW, 128), BF16),
            pltpu.VMEM((RAW, 128), F32),
            pltpu.VMEM((64 - RAW, 128), BF16),
            pltpu.VMEM((64, 128), BF16),
            pltpu.VMEM((2, 64, 128), BF16),
            pltpu.VMEM((6, 64, 128), F32),
            pltpu.VMEM((3, 64, 128), F32),
            pltpu.VMEM((8, 8, 128), jnp.int32),
            pltpu.SemaphoreType.DMA((1 + nc,)),
            pltpu.SemaphoreType.DMA((4,)),
            pltpu.SemaphoreType.DMA((3 + nc,)),
            pltpu.SemaphoreType.REGULAR((2,)),
            pltpu.SemaphoreType.REGULAR,
        ],
        compiler_params=pltpu.CompilerParams(
            collective_id=0, disable_bounds_checks=True, disable_semaphore_checks=True),
    )(x.T)
    return out_t.T
```

```python
import dataclasses

import jax
import jax.numpy as jnp
from jax import lax
from jax.experimental import pallas as pl
from jax.experimental.pallas import tpu as pltpu

F32 = jnp.float32
BF16 = jnp.bfloat16
U32 = jnp.uint32

RAW = 24
CHUNKS = ((24, 32), (32, 40), (40, 56), (56, 64))
SLOT = {(3, 0): 0, (1, 0): 1, (1, 2): 0, (3, 2): 1,
        (0, 1): 0, (2, 1): 1, (0, 3): 0, (2, 3): 1}
SORT8 = ((0, 2), (1, 3), (4, 6), (5, 7), (0, 4), (1, 5), (2, 6), (3, 7),
         (0, 1), (2, 3), (4, 5), (6, 7), (2, 4), (3, 5), (1, 4), (3, 6),
         (1, 2), (3, 4), (5, 6))


def _iotas():
    lane = lax.broadcasted_iota(jnp.int32, (8, 128), 1)
    sub = lax.broadcasted_iota(jnp.int32, (8, 128), 0)
    return lane, sub


def _vregs(v):
    return [v[8 * i:8 * i + 8, :] for i in range(v.shape[0] // 8)]


def _srot(x, k):
    return pltpu.roll(x, (8 - k) % 8, 0)


def _negate(xs, m):
    sign = jnp.where(m, -1.0, 1.0).astype(F32)
    return [x * sign for x in xs]


def _rot_v(g, t):
    for d in (1, 2, 4):
        m = (t & d) != 0
        g = [jnp.where(m, g[(j + d) % 8], g[j]) for j in range(8)]
    return g


def _rot_s(g, t):
    for d in (1, 2, 4):
        m = (t & d) != 0
        g = [jnp.where(m, _srot(x, d), x) for x in g]
    return g


def _rot_s_flat(g, t):
    out = []
    for x in g:
        c = [x] + [_srot(x, k) for k in range(1, 8)]
        for d in (1, 2, 4):
            m = (t & d) != 0
            c = [jnp.where(m, b, a) for a, b in zip(c[0::2], c[1::2])]
        out.append(c[0])
    return out


def _to_lanes_a(xs):
    lane, sub = _iotas()
    return _negate(_rot_s(xs, lane), (sub & 2) != 0)


def _to_lanes_b(xs):
    lane, sub = _iotas()
    xs = _rot_v(xs, (lane + sub) >> 3)
    return [pltpu.roll(x, 8 * i, 1, stride=1, stride_axis=0) for i, x in enumerate(xs)]


def _to_rows_pattern(j):
    lane, sub = _iotas()
    c_hi = (j + 1 + lane) & 7
    c_lo = (sub + 1 + (lane >> 3)) & 7
    return (lane & 64) | (c_hi << 3) | c_lo


def _to_rows(f, pat):
    lane, _ = _iotas()
    g = _rot_v(f, -(lane >> 3))
    g = [jnp.take_along_axis(g[j], pat[j], axis=1, mode="promise_in_bounds") for j in range(8)]
    return _rot_v(_rot_s_flat(g, -1 - (lane >> 3)), -1 - lane)


def _v_stage(xs, d, desc=False):
    xs = list(xs)
    for i in range(8):
        if i & d == 0:
            lo, hi = jnp.minimum(xs[i], xs[i + d]), jnp.maximum(xs[i], xs[i + d])
            xs[i], xs[i + d] = (hi, lo) if desc else (lo, hi)
    return xs


def _v_merge(xs, desc=False):
    for d in (4, 2, 1):
        xs = _v_stage(xs, d, desc)
    return xs


def _s_stage(xs, d, desc=False, mirror=False, skew=False):
    lane, sub = _iotas()
    upper = ((sub - lane if skew else sub) & d) != 0
    out = []
    for i, x in enumerate(xs):
        p = xs[7 - i] if mirror else x
        up = _srot(p, d)
        dn = up if d == 4 else _srot(p, 8 - d)
        if desc:
            out.append(jnp.where(upper, jnp.minimum(x, dn), jnp.maximum(x, up)))
        else:
            out.append(jnp.where(upper, jnp.maximum(x, dn), jnp.minimum(x, up)))
    return out


def _swap(xs, d):
    _, sub = _iotas()
    upper = (sub & d) != 0
    xs = list(xs)
    for i in range(4):
        a, b = xs[i], xs[i + 4]
        xs[i] = jnp.where(upper, _srot(b, 8 - d), a)
        xs[i + 4] = jnp.where(upper, b, _srot(a, d))
    return xs


def _bmerge(xs, desc=False, skew=False):
    for d in (4, 2, 1):
        xs = _s_stage(xs, d, desc, skew=skew)
    return _v_merge(xs, desc)


def _sort64_desc(xs):
    _, sub = _iotas()
    p0 = (sub & 1) != 0
    p1 = (sub & 2) != 0
    xs = list(xs)
    for i, j in SORT8:
        xs[i], xs[j] = jnp.minimum(xs[i], xs[j]), jnp.maximum(xs[i], xs[j])
    xs = _v_merge(_s_stage(xs, 4, mirror=True))
    xs = _negate(xs, p1 != p0)
    for d in (2, 4):
        xs = _v_stage(_swap(xs, d), 4)
    xs = _v_merge(_swap(xs, 2))
    xs = _negate(xs, p0)
    for d in (1, 4, 2):
        xs = _v_stage(_swap(xs, d), 4, True)
    return _v_merge(_swap(xs, 1), True)


def _clamp(run, lo, hi):
    return [jnp.maximum(l, jnp.minimum(h, x)) for x, l, h in zip(run, lo, hi)]


def _insert(blocks, run, first=False, last=False):
    out = []
    if first:
        out.append(_bmerge([jnp.minimum(x, h) for x, h in zip(run, blocks[0])]))
    for lo, hi in zip(blocks[:-1], blocks[1:]):
        out.append(_bmerge(_clamp(run, lo, hi)))
    if last:
        out.append(_bmerge([jnp.maximum(x, l) for x, l in zip(run, blocks[-1])]))
    return out


def _other_half(xs):
    return [pltpu.roll(x, 64, 1) for x in xs]


def _pack(xs):
    u = [lax.bitcast_convert_type(x, U32) for x in xs]
    return [(a & U32(0xFFFF0000)) | (b >> 16) for a, b in zip(u[0::2], u[1::2])]


def _unpack(ws):
    out = []
    for w in ws:
        out.append(lax.bitcast_convert_type(w & U32(0xFFFF0000), F32))
        out.append(lax.bitcast_convert_type(w << 16, F32))
    return out


def _body(x_hbm, o_ref, xv, send_b, recv_a, recv_b, send_s, recv_s, ext, win, pat,
          ld_sem, send_sem, recv_sem, up_sem, go_sem):
    me = lax.axis_index("i")
    bar = pltpu.get_barrier_semaphore()
    nc = len(CHUNKS)

    def load(lo, hi, i):
        rows = pl.ds(lo, hi - lo)
        return pltpu.make_async_copy(x_hbm.at[rows], xv.at[rows], ld_sem.at[i])

    def signal(sem, dev):
        pl.semaphore_signal(sem, inc=1, device_id=(dev,), device_id_type=pl.DeviceIdType.MESH)

    def remote(src, dst, s, r, dev):
        return pltpu.make_async_remote_copy(
            src, dst, send_sem.at[s], recv_sem.at[r],
            device_id=(dev,), device_id_type=pl.DeviceIdType.MESH)

    def cp_raw(dev):
        return remote(x_hbm.at[pl.ds(0, RAW)], recv_a, 0, 0, dev)

    def cp_chunk(dev, i):
        rows = pl.ds(CHUNKS[i][0] - RAW, CHUNKS[i][1] - CHUNKS[i][0])
        return remote(send_b.at[rows], recv_b.at[rows], 3, 3 + i, dev)

    def cp_sorted(src, dev):
        slot = SLOT[(src, dev)]
        return remote(send_s, recv_s.at[slot], 1 + (dev >> 1), 1 + slot, dev)

    def send_diagonal(dev):
        cp_raw(dev).start()
        for i in range(nc):
            cp_chunk(dev, i).start()

    def put(ref, i, block):
        ref[i] = jnp.concatenate(block, axis=0)

    load(*CHUNKS[0], 1).start()

    @pl.when(me == 2)
    def _():
        pl.semaphore_wait(bar, 1)
        cp_raw(0).start()
        signal(up_sem.at[1], 0)

    for i in range(1, nc):
        load(*CHUNKS[i], 1 + i).start(priority=1)

    @pl.when(me != 2)
    def _():
        load(0, RAW, 0).start()

    @pl.when(me == 0)
    def _():
        for dev in (2, 1, 3):
            signal(bar, dev)

    @pl.when((me & 1) == 1)
    def _():
        pl.semaphore_wait(bar, 1)
        signal(up_sem.at[0], 0)

    for i, (lo, hi) in enumerate(CHUNKS):
        load(lo, hi, 1 + i).wait()
        rows = xv[lo:hi, :]
        if i == nc - 1:
            rows = jnp.concatenate(_to_lanes_a(_vregs(rows)), axis=0)
        send_b[lo - RAW:hi - RAW, :] = rows.astype(BF16)

        @pl.when(me == 2)
        def _(i=i):
            cp_chunk(0, i).start()

    @pl.when(me == 2)
    def _():
        load(0, RAW, 0).start()

    load(0, RAW, 0).wait()
    own = _sort64_desc(_to_lanes_b(_to_lanes_a(_vregs(xv[...]))))
    send_s[...] = jnp.concatenate(own, axis=0).astype(BF16)

    for k in (1, 3):
        @pl.when(me == k)
        def _(k=k):
            cp_sorted(k, 0).start()

    mine = _insert([_bmerge(own)], _other_half(own), True, True)
    for j in range(8):
        pat[j] = _to_rows_pattern(j)
    lane, _ = _iotas()
    hi_half = lane >= 64

    @pl.when(me == 0)
    def _():
        pl.semaphore_wait(up_sem.at[0], 2)
        signal(bar, 2)
        signal(go_sem, 1)
        signal(go_sem, 3)
        cp_sorted(0, 1).start()
        cp_sorted(0, 3).start()
        pl.semaphore_wait(up_sem.at[1], 1)
        signal(up_sem.at[1], 1)
        signal(up_sem.at[1], 3)
        send_diagonal(2)

        cp_sorted(3, 0).wait_recv()
        cp_sorted(1, 0).wait_recv()
        b = _vregs(recv_s[0].astype(F32))
        c = _vregs(recv_s[1].astype(F32))
        st = mine
        for run in (b, c, _other_half(b), _other_half(c)):
            st = _insert(st, run, first=True)
        neg_inf = jnp.full((8, 128), -jnp.inf, F32)
        put(win, 0, [neg_inf] * 8)
        put(win, 1, [jnp.where(hi_half, x, neg_inf) for x in st[0]])
        put(win, 2, [jnp.where(hi_half, y, x) for x, y in zip(*st)])

    @pl.when(me != 0)
    def _():
        ext[0] = jnp.full((64, 128), -jnp.inf, F32)
        ext[5] = jnp.full((64, 128), jnp.inf, F32)
        for k in (1, 3):
            @pl.when(me == k)
            def _(k=k):
                pl.semaphore_wait(go_sem, 1)
                send_diagonal(4 - k)

        @pl.when(me == 2)
        def _():
            pl.semaphore_wait(bar, 1)
            cp_sorted(2, 1).start()
            cp_sorted(2, 3).start()

        cp_sorted(3, 0).wait_recv()
        b = _vregs(recv_s[0].astype(F32))
        st = _insert(_insert(mine, b, True, True), _other_half(b), True, True)
        for i, block in enumerate(st):
            put(ext, 1 + i, block)
        e = [_vregs(ext[jnp.clip(2 * me - 3 + t, 0, 5)]) for t in range(6)]
        st = [[jnp.where(hi_half, y, x) for x, y in zip(e[t], e[t + 1])] for t in range(5)]

        for k in (1, 3):
            @pl.when(me == k)
            def _(k=k):
                pl.semaphore_wait(up_sem.at[1], 1)
                cp_sorted(k, 2).start()

        cp_sorted(1, 0).wait_recv()
        c = _vregs(recv_s[1].astype(F32))
        st = _insert(_insert(st, c), _other_half(c))
        for i, block in enumerate(st):
            put(win, i, block)

    cp_raw(0).wait_recv()
    d = _to_lanes_a(_vregs(recv_a[...].astype(BF16).astype(F32)))
    cp_sorted(1, 0).wait_send()
    cp_sorted(1, 2).wait_send()
    cp_raw(0).wait_send()
    for i, (lo, hi) in enumerate(CHUNKS):
        if i == nc - 1:
            pltpu.make_async_copy(send_b, send_b, send_sem.at[3]).wait()
        cp_chunk(0, i).wait_recv()
        rows = _vregs(recv_b[lo - RAW:hi - RAW, :].astype(F32))
        d = d + (rows if i == nc - 1 else _to_lanes_a(rows))

    w = _pack(_sort64_desc(_to_lanes_b(d)))
    far = _unpack(_other_half(w))
    n0, n1 = _insert([_vregs(win[i]) for i in range(3)], _unpack(w))
    res = _to_rows(_bmerge(_clamp(far, n0, n1), desc=True, skew=True), pat)
    for j in range(8):
        o_ref[8 * j:8 * j + 8, :] = res[j]


def pallas_dist_sort_i_m128_n64_kernel(x: jax.Array):
    nc = len(CHUNKS)
    known = {f.name for f in dataclasses.fields(pltpu.CompilerParams)}
    no_asserts = {k: True for k in ("disable_bounds_checks", "disable_semaphore_checks") if k in known}
    out_t = pl.pallas_call(
        _body,
        out_shape=jax.ShapeDtypeStruct((64, 128), F32),
        in_specs=[pl.BlockSpec(memory_space=pl.ANY)],
        out_specs=pl.BlockSpec(memory_space=pltpu.VMEM),
        scratch_shapes=[
            pltpu.VMEM((64, 128), F32),
            pltpu.VMEM((64 - RAW, 128), BF16),
            pltpu.VMEM((RAW, 128), F32),
            pltpu.VMEM((64 - RAW, 128), BF16),
            pltpu.VMEM((64, 128), BF16),
            pltpu.VMEM((2, 64, 128), BF16),
            pltpu.VMEM((6, 64, 128), F32),
            pltpu.VMEM((3, 64, 128), F32),
            pltpu.VMEM((8, 8, 128), jnp.int32),
            pltpu.SemaphoreType.DMA((1 + nc,)),
            pltpu.SemaphoreType.DMA((4,)),
            pltpu.SemaphoreType.DMA((3 + nc,)),
            pltpu.SemaphoreType.REGULAR((2,)),
            pltpu.SemaphoreType.REGULAR,
        ],
        compiler_params=pltpu.CompilerParams(collective_id=0, **no_asserts),
    )(x.T)
    return out_t.T
```

```python
import dataclasses

import jax
import jax.numpy as jnp
from jax import lax
from jax.experimental import pallas as pl
from jax.experimental.pallas import tpu as pltpu

F32 = jnp.float32
BF16 = jnp.bfloat16

RAW = 24
CHUNKS = ((24, 32), (32, 40), (40, 56), (56, 64))
SLOT = {(3, 0): 0, (1, 0): 1, (1, 2): 0, (3, 2): 1,
        (0, 1): 0, (2, 1): 1, (0, 3): 0, (2, 3): 1}
SORT8 = ((0, 2), (1, 3), (4, 6), (5, 7), (0, 4), (1, 5), (2, 6), (3, 7),
         (0, 1), (2, 3), (4, 5), (6, 7), (2, 4), (3, 5), (1, 4), (3, 6),
         (1, 2), (3, 4), (5, 6))


def _iotas():
    lane = lax.broadcasted_iota(jnp.int32, (8, 128), 1)
    sub = lax.broadcasted_iota(jnp.int32, (8, 128), 0)
    return lane, sub


def _vregs(v):
    return [v[8 * i:8 * i + 8, :] for i in range(v.shape[0] // 8)]


def _gather(x, idx, axis):
    return jnp.take_along_axis(x, idx, axis=axis, mode="promise_in_bounds")


def _sxor(x, m):
    if m == 0:
        return x
    if m == 4:
        return pltpu.roll(x, 4, 0)
    return _gather(x, _iotas()[1] ^ m, 0)


def _rot_v(g, t):
    for d in (1, 2, 4):
        m = (t & d) != 0
        g = [jnp.where(m, g[(j + d) % 8], g[j]) for j in range(8)]
    return g


def _xor_v(g, t):
    for d in (1, 2, 4):
        m = (t & d) != 0
        g = [jnp.where(m, g[j ^ d], g[j]) for j in range(8)]
    return g


def _to_lanes_a(xs):
    lane, sub = _iotas()
    return [_gather(x, (sub + lane) & 7, 0) for x in xs]


def _to_lanes_b(xs, both=False):
    lane, sub = _iotas()
    xs = _rot_v(xs, (lane + sub) >> 3)
    out = [pltpu.roll(x, 8 * i, 1, stride=1, stride_axis=0) for i, x in enumerate(xs)]
    if both:
        out += [pltpu.roll(x, 8 * i + 64, 1, stride=1, stride_axis=0) for i, x in enumerate(xs)]
    return out


def _to_rows_pattern(j):
    lane, sub = _iotas()
    return (lane & 64) | (((lane ^ j) & 7) << 3) | ((sub ^ (lane >> 3)) & 7)


def _to_rows(f, pat):
    lane, sub = _iotas()
    g = _xor_v(f, lane >> 3)
    g = [_gather(g[j], pat[j], 1) for j in range(8)]
    g = [_gather(x, (sub ^ (lane >> 3)) & 7, 0) for x in g]
    return _xor_v(g, lane)


def _cx(xs, p, tv, ts=0, desc=False):
    out = list(xs)
    for v in range(8):
        if v & p == 0:
            a, b = xs[v], _sxor(xs[v ^ tv], ts)
            lo, hi = jnp.minimum(a, b), jnp.maximum(a, b)
            out[v], out[v | p] = (hi, lo) if desc else (lo, hi)
    return out


def _v_merge(xs):
    for d in (4, 2, 1):
        xs = _cx(xs, d, d)
    return xs


def _mix(xs, d):
    m = (_iotas()[1] & d) != 0
    return [jnp.where(m, xs[v ^ 4], xs[v]) for v in range(8)]


def _bmerge(xs, skew=False):
    lane, sub = _iotas()
    for d in (4, 2, 1):
        xs = _cx(_mix(xs, d), 4, 4, d)
    xs = _mix(xs, 4)
    dst = (sub ^ lane) & 7 if skew else sub
    src = ((dst & 1) << 2) | (dst >> 1)
    return _v_merge([_gather(x, src if v < 4 else src ^ 4, 0) for v, x in enumerate(xs)])


def _put_t(ref, i, xs):
    for v, x in enumerate(xs):
        ref[i, 9 * v:9 * v + 8, :] = x


def _get_t(ref, i):
    return [ref[i, pl.ds(j, 8, stride=9), :] for j in range(8)]


def _transpose(xs, ref, i):
    _put_t(ref, i, xs)
    return _get_t(ref, i)


def _merge_level(xs, new, old, desc=False):
    xs = _cx(xs, 4, 7, new + sum(old), desc)
    for d in old:
        xs = _cx(_mix(xs, d), 4, 4, d, desc)
    xs = _cx(_mix(xs, new), 4, 7, new, desc)
    return _cx(_cx(xs, 2, 2, 0, desc), 1, 1, 0, desc)


def _sort64_desc(xs):
    xs = list(xs)
    for i, j in SORT8:
        xs[i], xs[j] = jnp.minimum(xs[i], xs[j]), jnp.maximum(xs[i], xs[j])
    xs = _merge_level(xs, 4, ())
    xs = _merge_level(xs, 2, (4,))
    return _merge_level(xs, 1, (4, 2), True)


def _clamp(run, lo, hi):
    return [jnp.maximum(l, jnp.minimum(h, x)) for x, l, h in zip(run, lo, hi)]


def _insert(blocks, run, first=False, last=False):
    out = []
    if first:
        out.append(_bmerge([jnp.minimum(x, h) for x, h in zip(run, blocks[0])]))
    for lo, hi in zip(blocks[:-1], blocks[1:]):
        out.append(_bmerge(_clamp(run, lo, hi)))
    if last:
        out.append(_bmerge([jnp.maximum(x, l) for x, l in zip(run, blocks[-1])]))
    return out


def _other_half(xs):
    return [pltpu.roll(x, 64, 1) for x in xs]


def _body(x_hbm, o_ref, xv, send_b, recv_a, recv_b, send_s, recv_s, ext, win, pat, tmp,
          ld_sem, send_sem, recv_sem, up_sem, go_sem):
    me = lax.axis_index("i")
    bar = pltpu.get_barrier_semaphore()
    nc = len(CHUNKS)

    def load(lo, hi, i):
        rows = pl.ds(lo, hi - lo)
        return pltpu.make_async_copy(x_hbm.at[rows], xv.at[rows], ld_sem.at[i])

    def signal(sem, dev):
        pl.semaphore_signal(sem, inc=1, device_id=(dev,), device_id_type=pl.DeviceIdType.MESH)

    def remote(src, dst, s, r, dev):
        return pltpu.make_async_remote_copy(
            src, dst, send_sem.at[s], recv_sem.at[r],
            device_id=(dev,), device_id_type=pl.DeviceIdType.MESH)

    def cp_raw(dev):
        return remote(x_hbm.at[pl.ds(0, RAW)], recv_a, 0, 0, dev)

    def cp_chunk(dev, i):
        rows = pl.ds(CHUNKS[i][0] - RAW, CHUNKS[i][1] - CHUNKS[i][0])
        return remote(send_b.at[rows], recv_b.at[rows], 3, 3 + i, dev)

    def cp_sorted(src, dev):
        slot = SLOT[(src, dev)]
        return remote(send_s, recv_s.at[slot], 1 + (dev >> 1), 1 + slot, dev)

    def send_diagonal(dev):
        cp_raw(dev).start()
        for i in range(nc):
            cp_chunk(dev, i).start()

    def put(ref, i, block):
        ref[i] = jnp.concatenate(block, axis=0)

    load(*CHUNKS[0], 1).start()

    @pl.when(me == 2)
    def _():
        pl.semaphore_wait(bar, 1)
        cp_raw(0).start()
        signal(up_sem.at[1], 0)

    for i in range(1, nc):
        load(*CHUNKS[i], 1 + i).start(priority=1)

    @pl.when(me != 2)
    def _():
        load(0, RAW, 0).start()

    @pl.when(me == 0)
    def _():
        for dev in (2, 1, 3):
            signal(bar, dev)

    @pl.when((me & 1) == 1)
    def _():
        pl.semaphore_wait(bar, 1)
        signal(up_sem.at[0], 0)

    for i, (lo, hi) in enumerate(CHUNKS):
        load(lo, hi, 1 + i).wait()
        rows = xv[lo:hi, :]
        if i == nc - 1:
            rows = jnp.concatenate(_to_lanes_a(_vregs(rows)), axis=0)
        send_b[lo - RAW:hi - RAW, :] = rows.astype(BF16)

        @pl.when(me == 2)
        def _(i=i):
            cp_chunk(0, i).start()

    @pl.when(me == 2)
    def _():
        load(0, RAW, 0).start()

    load(0, RAW, 0).wait()
    own = _sort64_desc(_to_lanes_b(_to_lanes_a(_vregs(xv[...]))))
    send_s[...] = jnp.concatenate(own, axis=0).astype(BF16)

    for k in (1, 3):
        @pl.when(me == k)
        def _(k=k):
            cp_sorted(k, 0).start()

    mine = _insert([_bmerge(own)], _other_half(own), True, True)
    for j in range(8):
        pat[j] = _to_rows_pattern(j)
    lane, _ = _iotas()
    hi_half = lane >= 64

    @pl.when(me == 0)
    def _():
        pl.semaphore_wait(up_sem.at[0], 2)
        signal(bar, 2)
        signal(go_sem, 1)
        signal(go_sem, 3)
        cp_sorted(0, 1).start()
        cp_sorted(0, 3).start()
        pl.semaphore_wait(up_sem.at[1], 1)
        signal(up_sem.at[1], 1)
        signal(up_sem.at[1], 3)
        send_diagonal(2)

        cp_sorted(3, 0).wait_recv()
        cp_sorted(1, 0).wait_recv()
        b = _vregs(recv_s[0].astype(F32))
        c = _vregs(recv_s[1].astype(F32))
        st = mine
        for run in (b, c, _other_half(b), _other_half(c)):
            st = _insert(st, run, first=True)
        neg_inf = jnp.full((8, 128), -jnp.inf, F32)
        _put_t(win, 0, [neg_inf] * 8)
        _put_t(win, 1, [jnp.where(hi_half, x, neg_inf) for x in st[0]])
        _put_t(win, 2, [jnp.where(hi_half, y, x) for x, y in zip(*st)])

    @pl.when(me != 0)
    def _():
        ext[0] = jnp.full((64, 128), -jnp.inf, F32)
        ext[5] = jnp.full((64, 128), jnp.inf, F32)
        for k in (1, 3):
            @pl.when(me == k)
            def _(k=k):
                pl.semaphore_wait(go_sem, 1)
                send_diagonal(4 - k)

        @pl.when(me == 2)
        def _():
            pl.semaphore_wait(bar, 1)
            cp_sorted(2, 1).start()
            cp_sorted(2, 3).start()

        cp_sorted(3, 0).wait_recv()
        b = _vregs(recv_s[0].astype(F32))
        st = _insert(_insert(mine, b, True, True), _other_half(b), True, True)
        for i, block in enumerate(st):
            put(ext, 1 + i, block)
        e = [_vregs(ext[jnp.clip(2 * me - 3 + t, 0, 5)]) for t in range(6)]
        st = [[jnp.where(hi_half, y, x) for x, y in zip(e[t], e[t + 1])] for t in range(5)]

        for k in (1, 3):
            @pl.when(me == k)
            def _(k=k):
                pl.semaphore_wait(up_sem.at[1], 1)
                cp_sorted(k, 2).start()

        cp_sorted(1, 0).wait_recv()
        c = _vregs(recv_s[1].astype(F32))
        st = _insert(_insert(st, c), _other_half(c))
        for i, block in enumerate(st):
            _put_t(win, i, block)

    cp_raw(0).wait_recv()
    d = _to_lanes_a(_vregs(recv_a[...]))
    cp_sorted(1, 0).wait_send()
    cp_sorted(1, 2).wait_send()
    cp_raw(0).wait_send()
    for i, (lo, hi) in enumerate(CHUNKS):
        if i == nc - 1:
            pltpu.make_async_copy(send_b, send_b, send_sem.at[3]).wait()
        cp_chunk(0, i).wait_recv()
        rows = _vregs(recv_b[lo - RAW:hi - RAW, :].astype(F32))
        d = d + (rows if i == nc - 1 else _to_lanes_a(rows))

    d = _to_lanes_b(d, True)
    near, far = _sort64_desc(d[:8]), _sort64_desc(d[8:])
    near = _transpose(near, tmp, 0)
    m = [_get_t(win, i) for i in range(3)]
    n0, n1 = [_v_merge(_transpose(_v_merge(_clamp(near, m[i], m[i + 1])), tmp, 1 + i)) for i in range(2)]
    res = _to_rows(_bmerge(_clamp(far, n0, n1), skew=True), pat)
    for j in range(8):
        o_ref[8 * j:8 * j + 8, :] = res[j]


def pallas_dist_sort_i_m128_n64_kernel(x: jax.Array):
    nc = len(CHUNKS)
    known = {f.name for f in dataclasses.fields(pltpu.CompilerParams)}
    no_asserts = {k: True for k in ("disable_bounds_checks", "disable_semaphore_checks") if k in known}
    out_t = pl.pallas_call(
        _body,
        out_shape=jax.ShapeDtypeStruct((64, 128), F32),
        in_specs=[pl.BlockSpec(memory_space=pl.ANY)],
        out_specs=pl.BlockSpec(memory_space=pltpu.VMEM),
        scratch_shapes=[
            pltpu.VMEM((64, 128), F32),
            pltpu.VMEM((64 - RAW, 128), BF16),
            pltpu.VMEM((RAW, 128), F32),
            pltpu.VMEM((64 - RAW, 128), BF16),
            pltpu.VMEM((64, 128), BF16),
            pltpu.VMEM((2, 64, 128), BF16),
            pltpu.VMEM((6, 64, 128), F32),
            pltpu.VMEM((3, 80, 128), F32),
            pltpu.VMEM((8, 8, 128), jnp.int32),
            pltpu.VMEM((3, 80, 128), F32),
            pltpu.SemaphoreType.DMA((1 + nc,)),
            pltpu.SemaphoreType.DMA((4,)),
            pltpu.SemaphoreType.DMA((3 + nc,)),
            pltpu.SemaphoreType.REGULAR((2,)),
            pltpu.SemaphoreType.REGULAR,
        ],
        compiler_params=pltpu.CompilerParams(collective_id=0, **no_asserts),
    )(x.T)
    return out_t.T
```
